```python
import numpy as np

kernel_name = "dist_rope_attn_htp_bs_b2_sq512_d1024_hq8_dh128"

def setup_inputs():
    x = np.random.randn(8, 512, 1024).astype(np.float32)
    Wq = np.random.randn(1024, 4096).astype(np.float32) * 0.02
    Wk = np.random.randn(1024, 4096).astype(np.float32) * 0.02
    Wv = np.random.randn(1024, 4096).astype(np.float32) * 0.02
    Wo = np.random.randn(4096, 1024).astype(np.float32) * 0.02
    return {"x": x, "Wq": Wq, "Wk": Wk, "Wv": Wv, "Wo": Wo}

def reference(x, Wq, Wk, Wv, Wo):
    B, Sq, Hq, Dh = 8, 512, 32, 128
    inv = 1.0 / (10000.0 ** (np.arange(0, Dh, 2) / Dh))
    pos = np.arange(Sq)[:, None] * inv[None, :]
    cos = np.repeat(np.cos(pos), 2, axis=-1).astype(np.float32)
    sin = np.repeat(np.sin(pos), 2, axis=-1).astype(np.float32)
    def rot(t):
        t2 = t.reshape(B, Sq, Hq, Dh // 2, 2)
        t_r = np.stack([-t2[..., 1], t2[..., 0]], axis=-1).reshape(B, Sq, Hq, Dh)
        return t * cos[None, :, None, :] + t_r * sin[None, :, None, :]
    Q = rot((x @ Wq).reshape(B, Sq, Hq, Dh))
    K = rot((x @ Wk).reshape(B, Sq, Hq, Dh))
    V = (x @ Wv).reshape(B, Sq, Hq, Dh)
    s = np.einsum('bihd,bjhd->bhij', Q, K).astype(np.float32) * 0.08838834764831843
    s_max = s.max(axis=-1, keepdims=True)
    w = np.exp(s - s_max)
    w = w / w.sum(axis=-1, keepdims=True)
    ctx = np.einsum('bhij,bjhd->bihd', w, V).reshape(B, Sq, Hq * Dh)
    return ctx @ Wo
```

```python
import numpy as np
import jax
import jax.numpy as jnp
from jax import lax
from jax.experimental import pallas as pl
from jax.experimental.pallas import tpu as pltpu

N_DEV = 4
B_LOC = 2
SQ = 512
D = 1024
H_LOC = 8
DH = 128
SCALE = 0.08838834764831843


def _rope_tables():
    inv = 1.0 / (10000.0 ** (np.arange(0, DH, 2) / DH))
    pos = np.arange(SQ)[:, None] * inv[None, :]
    cos = np.repeat(np.cos(pos), 2, axis=-1)
    sin = np.repeat(np.sin(pos), 2, axis=-1)
    sign = np.where(np.arange(DH) % 2 == 0, -1.0, 1.0)[None, :]
    sin_s = sin * sign
    tab = np.stack([cos, sin_s, cos * SCALE, sin_s * SCALE]).astype(np.float32)
    return tab


def _rope(t, cos, sin_s, even):
    t_next = pltpu.roll(t, DH - 1, 1)
    t_prev = pltpu.roll(t, 1, 1)
    tr = jnp.where(even, t_next, t_prev)
    return t * cos + tr * sin_s


def pallas_dist_rope_attn_htp_bs_b2_sq512_d1024_hq8_dh128_kernel(x, Wq, Wk, Wv, Wo):
    tab = jnp.asarray(_rope_tables())

    def body(x_hbm, wq_hbm, wk_hbm, wv_hbm, wo_hbm, tab_ref, out_ref,
             xstage, xg, wstage, wqkv, wo, sendbuf, recvbuf,
             ld_sems, ag_send, ag_recv, rs_send, rs_recv):
        me = lax.axis_index("i")


        xcp = pltpu.make_async_copy(x_hbm, xstage, ld_sems.at[0])
        xcp.start()
        w_hbm = [wq_hbm, wk_hbm, wv_hbm, wo_hbm]
        wcps = [pltpu.make_async_copy(w_hbm[j], wstage.at[j], ld_sems.at[1 + j]) for j in range(4)]
        for c in wcps:
            c.start()
        xcp.wait()
        for b in range(B_LOC):
            xg[me, b] = xstage[b].astype(jnp.bfloat16)

        def ag_copy(d, b):
            return pltpu.make_async_remote_copy(
                src_ref=xg.at[me, b], dst_ref=xg.at[me, b],
                send_sem=ag_send.at[(d - 1) * 2 + b],
                recv_sem=ag_recv.at[(N_DEV - d - 1) * 2 + b],
                device_id=((me + d) % N_DEV,), device_id_type=pl.DeviceIdType.MESH)
        for b in range(B_LOC):
            for d in (3, 1, 2):
                ag_copy(d, b).start()

        for j in range(3):
            wcps[j].wait()
            wqkv[:, j * D:(j + 1) * D] = wstage[j].astype(jnp.bfloat16)
        wcps[3].wait()
        wo[...] = wstage[3].astype(jnp.bfloat16)

        lane = lax.broadcasted_iota(jnp.int32, (SQ, DH), 1)
        even = (lane % 2) == 0

        def step(s, carry):
            r = s - 1
            q = r // 2
            remote = jnp.logical_and(s >= 1, s <= 6)
            d = jnp.where(remote, 1 + 2 * q - 3 * (q == 2).astype(jnp.int32), 0)
            b = jnp.where(remote, r % 2, jnp.where(s == 0, 0, 1))
            src = (me + d) % N_DEV
            ridx = (d - 1) * 2 + b

            @pl.when(remote)
            def _():
                pltpu.make_async_remote_copy(
                    src_ref=xg.at[src, b], dst_ref=xg.at[src, b],
                    send_sem=ag_send.at[0], recv_sem=ag_recv.at[ridx],
                    device_id=(src,), device_id_type=pl.DeviceIdType.MESH).wait_recv()

            xb = xg[src, b]
            qkv = jnp.dot(xb, wqkv[...], preferred_element_type=jnp.float32)
            cos_k = tab_ref[0]
            sin_k = tab_ref[1]
            cos_q = tab_ref[2]
            sin_q = tab_ref[3]
            ctxs = []
            for h in range(H_LOC):
                qh = _rope(qkv[:, h * DH:(h + 1) * DH], cos_q, sin_q, even).astype(jnp.bfloat16)
                kh = _rope(qkv[:, D + h * DH:D + (h + 1) * DH], cos_k, sin_k, even).astype(jnp.bfloat16)
                vh = qkv[:, 2 * D + h * DH:2 * D + (h + 1) * DH].astype(jnp.bfloat16)
                sc = lax.dot_general(qh, kh, (((1,), (1,)), ((), ())),
                                     preferred_element_type=jnp.float32)
                m = jnp.max(sc, axis=-1, keepdims=True)
                p = jnp.exp(sc - m)
                l = jnp.sum(p, axis=-1, keepdims=True)
                o = jnp.dot(p.astype(jnp.bfloat16), vh, preferred_element_type=jnp.float32)
                ctxs.append((o / l).astype(jnp.bfloat16))
            ctx = jnp.concatenate(ctxs, axis=1)
            part = jnp.dot(ctx, wo[...], preferred_element_type=jnp.float32)

            @pl.when(remote)
            def _():
                sendbuf[ridx] = part.astype(jnp.bfloat16)
                oidx = (N_DEV - d - 1) * 2 + b
                pltpu.make_async_remote_copy(
                    src_ref=sendbuf.at[ridx], dst_ref=recvbuf.at[oidx],
                    send_sem=rs_send.at[ridx], recv_sem=rs_recv.at[oidx],
                    device_id=(src,), device_id_type=pl.DeviceIdType.MESH).start()

            @pl.when(jnp.logical_not(remote))
            def _():
                out_ref[b] = part
            return carry

        lax.fori_loop(0, 8, step, 0)

        for i in range(6):
            pltpu.make_async_remote_copy(
                src_ref=sendbuf.at[i], dst_ref=recvbuf.at[i],
                send_sem=rs_send.at[i], recv_sem=rs_recv.at[i],
                device_id=(me,), device_id_type=pl.DeviceIdType.MESH).wait_recv()
        for b in range(B_LOC):
            out_ref[b] = (out_ref[b]
                          + recvbuf[0 + b].astype(jnp.float32)
                          + recvbuf[2 + b].astype(jnp.float32)
                          + recvbuf[4 + b].astype(jnp.float32))
        for i in range(6):
            pltpu.make_async_remote_copy(
                src_ref=sendbuf.at[i], dst_ref=recvbuf.at[i],
                send_sem=rs_send.at[i], recv_sem=rs_recv.at[i],
                device_id=(me,), device_id_type=pl.DeviceIdType.MESH).wait_send()
        for b in range(B_LOC):
            for d in (1, 2, 3):
                ag_copy(d, b).wait_send()

    return pl.pallas_call(
        body,
        out_shape=jax.ShapeDtypeStruct((B_LOC, SQ, D), jnp.float32),
        in_specs=[pl.BlockSpec(memory_space=pl.ANY)] * 5 + [pl.BlockSpec(memory_space=pltpu.VMEM)],
        out_specs=pl.BlockSpec(memory_space=pltpu.VMEM),
        scratch_shapes=[
            pltpu.VMEM((B_LOC, SQ, D), jnp.float32),
            pltpu.VMEM((N_DEV, B_LOC, SQ, D), jnp.bfloat16),
            pltpu.VMEM((4, D, D), jnp.float32),
            pltpu.VMEM((D, 3 * D), jnp.bfloat16),
            pltpu.VMEM((D, D), jnp.bfloat16),
            pltpu.VMEM((6, SQ, D), jnp.bfloat16),
            pltpu.VMEM((6, SQ, D), jnp.bfloat16),
            pltpu.SemaphoreType.DMA((5,)),
            pltpu.SemaphoreType.DMA((6,)),
            pltpu.SemaphoreType.DMA((6,)),
            pltpu.SemaphoreType.DMA((6,)),
            pltpu.SemaphoreType.DMA((6,)),
        ],
        compiler_params=pltpu.CompilerParams(vmem_limit_bytes=110 * 1024 * 1024),
    )(x, Wq, Wk, Wv, Wo, tab)
```

```python
import math
import jax
import jax.numpy as jnp
from jax import lax
from jax.experimental import pallas as pl
from jax.experimental.pallas import tpu as pltpu

N_DEV = 4
B_LOC = 2
SQ = 512
D = 1024
H_LOC = 8
DH = 128
SCALE = 0.08838834764831843


def _rope(t, cos, sin_s, even):
    t_next = pltpu.roll(t, DH - 1, 1)
    t_prev = pltpu.roll(t, 1, 1)
    tr = jnp.where(even, t_next, t_prev)
    return t * cos + tr * sin_s


def pallas_dist_rope_attn_htp_bs_b2_sq512_d1024_hq8_dh128_kernel(x, Wq, Wk, Wv, Wo):

    def body(x_hbm, wq_hbm, wk_hbm, wv_hbm, wo_hbm, out_hbm,
             xstage, xg, wstage, wbf, tab, sendbuf, recvbuf,
             ld_sems, ag_send, ag_recv, rs_send, rs_recv):
        me = lax.axis_index("i")
        acc = out_hbm
        w_hbm = [wq_hbm, wk_hbm, wv_hbm, wo_hbm]

        xcps = [pltpu.make_async_copy(x_hbm.at[b], xstage.at[b], ld_sems.at[b]) for b in range(B_LOC)]
        wcps = [pltpu.make_async_copy(w_hbm[j], wstage.at[j], ld_sems.at[2 + j]) for j in range(4)]

        def ag_copy(d, b):
            return pltpu.make_async_remote_copy(
                src_ref=xg.at[me, b], dst_ref=xg.at[me, b],
                send_sem=ag_send.at[(d - 1) * 2 + b],
                recv_sem=ag_recv.at[(N_DEV - d - 1) * 2 + b],
                device_id=((me + d) % N_DEV,), device_id_type=pl.DeviceIdType.MESH)

        xcps[0].start()
        wcps[0].start()

        lane = lax.broadcasted_iota(jnp.int32, (SQ, DH), 1)
        row = lax.broadcasted_iota(jnp.int32, (SQ, DH), 0)
        even = (lane % 2) == 0
        inv = jnp.exp((lane // 2).astype(jnp.float32) * (-2.0 * math.log(10000.0) / DH))
        ang = row.astype(jnp.float32) * inv
        c = jnp.cos(ang)
        s_ = jnp.where(even, -1.0, 1.0) * jnp.sin(ang)
        tab[0] = c
        tab[1] = s_
        tab[2] = c * SCALE
        tab[3] = s_ * SCALE

        xcps[0].wait()
        xcps[1].start()
        for j in range(1, 4):
            wcps[j].start()
        xg[me, 0] = xstage[0].astype(jnp.bfloat16)
        ag_copy(3, 0).start()
        ag_copy(1, 0).start()

        def wcast(j):
            wcps[j].wait()
            wbf[j] = wstage[j].astype(jnp.bfloat16)

        def rs_wait(i):
            pltpu.make_async_remote_copy(
                src_ref=sendbuf.at[i], dst_ref=recvbuf.at[i],
                send_sem=rs_send.at[i], recv_sem=rs_recv.at[i],
                device_id=(me,), device_id_type=pl.DeviceIdType.MESH).wait_recv()

        def finalize(b):
            for i in range(3):
                rs_wait(2 * i + b)
            acc[b] = (acc[b]
                      + recvbuf[0 + b].astype(jnp.float32)
                      + recvbuf[2 + b].astype(jnp.float32)
                      + recvbuf[4 + b].astype(jnp.float32))

        def step(s, carry):
            r = s - 1
            q = r // 2
            remote = jnp.logical_and(s >= 1, s <= 6)
            first = s == 0
            d = jnp.where(remote, 1 + 2 * q - 3 * (q == 2).astype(jnp.int32), 0)
            b = jnp.where(remote, r % 2, jnp.where(first, 0, 1))
            src = (me + d) % N_DEV
            ridx = (d - 1) * 2 + b

            @pl.when(remote)
            def _():
                pltpu.make_async_remote_copy(
                    src_ref=xg.at[src, b], dst_ref=xg.at[src, b],
                    send_sem=ag_send.at[0], recv_sem=ag_recv.at[ridx],
                    device_id=(src,), device_id_type=pl.DeviceIdType.MESH).wait_recv()

            @pl.when(s == 7)
            def _():
                finalize(0)

            xb = xg[src, b]

            @pl.when(first)
            def _():
                wcast(0)
            qa = jnp.dot(xb, wbf[0], preferred_element_type=jnp.float32)

            @pl.when(first)
            def _():
                xcps[1].wait()
                xg[me, 1] = xstage[1].astype(jnp.bfloat16)
                ag_copy(3, 1).start()
                ag_copy(1, 1).start()
                wcast(1)
            ka = jnp.dot(xb, wbf[1], preferred_element_type=jnp.float32)

            @pl.when(first)
            def _():
                wcast(2)
            va = jnp.dot(xb, wbf[2], preferred_element_type=jnp.float32)

            cos_k = tab[0]
            sin_k = tab[1]
            cos_q = tab[2]
            sin_q = tab[3]
            ctxs = []
            for h in range(H_LOC):
                qh = _rope(qa[:, h * DH:(h + 1) * DH], cos_q, sin_q, even).astype(jnp.bfloat16)
                kh = _rope(ka[:, h * DH:(h + 1) * DH], cos_k, sin_k, even).astype(jnp.bfloat16)
                vh = va[:, h * DH:(h + 1) * DH].astype(jnp.bfloat16)
                sc = lax.dot_general(qh, kh, (((1,), (1,)), ((), ())),
                                     preferred_element_type=jnp.float32)
                m = jnp.max(sc, axis=-1, keepdims=True)
                p = jnp.exp(sc - m)
                l = jnp.sum(p, axis=-1, keepdims=True)
                o = jnp.dot(p.astype(jnp.bfloat16), vh, preferred_element_type=jnp.float32)
                ctxs.append((o / l).astype(jnp.bfloat16))
            ctx = jnp.concatenate(ctxs, axis=1)

            @pl.when(first)
            def _():
                ag_copy(2, 0).start()
                ag_copy(2, 1).start()
                wcast(3)
            part = jnp.dot(ctx, wbf[3], preferred_element_type=jnp.float32)

            @pl.when(remote)
            def _():
                sendbuf[ridx] = part.astype(jnp.bfloat16)
                oidx = (N_DEV - d - 1) * 2 + b
                pltpu.make_async_remote_copy(
                    src_ref=sendbuf.at[ridx], dst_ref=recvbuf.at[oidx],
                    send_sem=rs_send.at[ridx], recv_sem=rs_recv.at[oidx],
                    device_id=(src,), device_id_type=pl.DeviceIdType.MESH).start()

            @pl.when(jnp.logical_not(remote))
            def _():
                acc[b] = part
            return carry

        lax.fori_loop(0, 8, step, 0)

        finalize(1)
        for i in range(6):
            pltpu.make_async_remote_copy(
                src_ref=sendbuf.at[i], dst_ref=recvbuf.at[i],
                send_sem=rs_send.at[i], recv_sem=rs_recv.at[i],
                device_id=(me,), device_id_type=pl.DeviceIdType.MESH).wait_send()
        for b in range(B_LOC):
            for d in (1, 2, 3):
                ag_copy(d, b).wait_send()

    return pl.pallas_call(
        body,
        out_shape=jax.ShapeDtypeStruct((B_LOC, SQ, D), jnp.float32),
        in_specs=[pl.BlockSpec(memory_space=pl.ANY)] * 5,
        out_specs=pl.BlockSpec(memory_space=pltpu.VMEM),
        scratch_shapes=[
            pltpu.VMEM((B_LOC, SQ, D), jnp.float32),
            pltpu.VMEM((N_DEV, B_LOC, SQ, D), jnp.bfloat16),
            pltpu.VMEM((4, D, D), jnp.float32),
            pltpu.VMEM((4, D, D), jnp.bfloat16),
            pltpu.VMEM((4, SQ, DH), jnp.float32),
            pltpu.VMEM((6, SQ, D), jnp.bfloat16),
            pltpu.VMEM((6, SQ, D), jnp.bfloat16),
            pltpu.SemaphoreType.DMA((6,)),
            pltpu.SemaphoreType.DMA((6,)),
            pltpu.SemaphoreType.DMA((6,)),
            pltpu.SemaphoreType.DMA((6,)),
            pltpu.SemaphoreType.DMA((6,)),
        ],
        compiler_params=pltpu.CompilerParams(vmem_limit_bytes=110 * 1024 * 1024),
    )(x, Wq, Wk, Wv, Wo)
```

```python
import math
import jax
import jax.numpy as jnp
from jax import lax
from jax.experimental import pallas as pl
from jax.experimental.pallas import tpu as pltpu

N_DEV = 4
B_LOC = 2
SQ = 512
D = 1024
H_LOC = 8
DH = 128
SCALE = 0.08838834764831843


def _rope(t, cos, sin_s, even):
    t_next = pltpu.roll(t, DH - 1, 1)
    t_prev = pltpu.roll(t, 1, 1)
    tr = jnp.where(even, t_next, t_prev)
    return t * cos + tr * sin_s


def pallas_dist_rope_attn_htp_bs_b2_sq512_d1024_hq8_dh128_kernel(x, Wq, Wk, Wv, Wo):
    def body(x_hbm, wq_hbm, wk_hbm, wv_hbm, wo_hbm, out_ref,
             xstage, xg, wstage, wbf, tab, sendbuf, recvbuf,
             ld_sems, ag_send, ag_recv, rs_send, rs_recv):
        me = lax.axis_index("i")
        w_hbm = [wq_hbm, wk_hbm, wv_hbm, wo_hbm]

        xcps = [pltpu.make_async_copy(x_hbm.at[b], xstage.at[b], ld_sems.at[b]) for b in range(B_LOC)]
        wcps = [pltpu.make_async_copy(w_hbm[j], wstage.at[j], ld_sems.at[2 + j]) for j in range(4)]

        def ag_copy(d, b):
            return pltpu.make_async_remote_copy(
                src_ref=xg.at[me, b], dst_ref=xg.at[me, b],
                send_sem=ag_send.at[(d - 1) * 2 + b],
                recv_sem=ag_recv.at[(N_DEV - d - 1) * 2 + b],
                device_id=((me + d) % N_DEV,), device_id_type=pl.DeviceIdType.MESH)

        xcps[0].start()
        wcps[0].start()

        lane = lax.broadcasted_iota(jnp.int32, (SQ, DH), 1)
        row = lax.broadcasted_iota(jnp.int32, (SQ, DH), 0)
        even = (lane % 2) == 0
        inv = jnp.exp((lane // 2).astype(jnp.float32) * (-2.0 * math.log(10000.0) / DH))
        ang = row.astype(jnp.float32) * inv
        c = jnp.cos(ang)
        s_ = jnp.where(even, -1.0, 1.0) * jnp.sin(ang)
        tab[0] = c
        tab[1] = s_
        tab[2] = c * SCALE
        tab[3] = s_ * SCALE

        xcps[0].wait()
        xcps[1].start()
        for j in range(1, 4):
            wcps[j].start()
        xg[me, 0] = xstage[0].astype(jnp.bfloat16)
        ag_copy(3, 0).start()
        ag_copy(1, 0).start()

        def wcast(j):
            wcps[j].wait()
            wbf[j] = wstage[j].astype(jnp.bfloat16)

        def rs_wait(i):
            pltpu.make_async_remote_copy(
                src_ref=sendbuf.at[i], dst_ref=recvbuf.at[i],
                send_sem=rs_send.at[i], recv_sem=rs_recv.at[i],
                device_id=(me,), device_id_type=pl.DeviceIdType.MESH).wait_recv()

        def finalize(b):
            for i in range(3):
                rs_wait(2 * i + b)
            out_ref[b] = (sendbuf[6 + b].astype(jnp.float32)
                          + recvbuf[0 + b].astype(jnp.float32)
                          + recvbuf[2 + b].astype(jnp.float32)
                          + recvbuf[4 + b].astype(jnp.float32))

        def step(s, carry):
            r = s - 1
            q = r // 2
            remote = jnp.logical_and(s >= 1, s <= 6)
            first = s == 0
            d = jnp.where(remote, 1 + 2 * q - 3 * (q == 2).astype(jnp.int32), 0)
            b = jnp.where(remote, r % 2, jnp.where(first, 0, 1))
            src = (me + d) % N_DEV
            ridx = (d - 1) * 2 + b

            @pl.when(remote)
            def _():
                pltpu.make_async_remote_copy(
                    src_ref=xg.at[src, b], dst_ref=xg.at[src, b],
                    send_sem=ag_send.at[0], recv_sem=ag_recv.at[ridx],
                    device_id=(src,), device_id_type=pl.DeviceIdType.MESH).wait_recv()

            @pl.when(s == 7)
            def _():
                finalize(0)

            xb = xg[src, b]

            @pl.when(first)
            def _():
                wcast(0)
            qa = jnp.dot(xb, wbf[0], preferred_element_type=jnp.float32)

            @pl.when(first)
            def _():
                xcps[1].wait()
                xg[me, 1] = xstage[1].astype(jnp.bfloat16)
                ag_copy(3, 1).start()
                ag_copy(1, 1).start()
                wcast(1)
            ka = jnp.dot(xb, wbf[1], preferred_element_type=jnp.float32)

            @pl.when(first)
            def _():
                wcast(2)
            va = jnp.dot(xb, wbf[2], preferred_element_type=jnp.float32)

            cos_k = tab[0]
            sin_k = tab[1]
            cos_q = tab[2]
            sin_q = tab[3]
            ctxs = []
            for h in range(H_LOC):
                qh = _rope(qa[:, h * DH:(h + 1) * DH], cos_q, sin_q, even).astype(jnp.bfloat16)
                kh = _rope(ka[:, h * DH:(h + 1) * DH], cos_k, sin_k, even).astype(jnp.bfloat16)
                vh = va[:, h * DH:(h + 1) * DH].astype(jnp.bfloat16)
                sc = lax.dot_general(qh, kh, (((1,), (1,)), ((), ())),
                                     preferred_element_type=jnp.float32)
                m = jnp.max(sc, axis=-1, keepdims=True)
                p = jnp.exp(sc - m)
                l = jnp.sum(p, axis=-1, keepdims=True)
                o = jnp.dot(p.astype(jnp.bfloat16), vh, preferred_element_type=jnp.float32)
                ctxs.append((o / l).astype(jnp.bfloat16))
            ctx = jnp.concatenate(ctxs, axis=1)

            @pl.when(first)
            def _():
                ag_copy(2, 0).start()
                ag_copy(2, 1).start()
                wcast(3)
            part = jnp.dot(ctx, wbf[3], preferred_element_type=jnp.float32)

            sidx = jnp.where(remote, ridx, 6 + b)
            sendbuf[sidx] = part.astype(jnp.bfloat16)

            @pl.when(remote)
            def _():
                oidx = (N_DEV - d - 1) * 2 + b
                pltpu.make_async_remote_copy(
                    src_ref=sendbuf.at[ridx], dst_ref=recvbuf.at[oidx],
                    send_sem=rs_send.at[ridx], recv_sem=rs_recv.at[oidx],
                    device_id=(src,), device_id_type=pl.DeviceIdType.MESH).start()

            return carry

        lax.fori_loop(0, 8, step, 0)

        finalize(1)
        for i in range(6):
            pltpu.make_async_remote_copy(
                src_ref=sendbuf.at[i], dst_ref=recvbuf.at[i],
                send_sem=rs_send.at[i], recv_sem=rs_recv.at[i],
                device_id=(me,), device_id_type=pl.DeviceIdType.MESH).wait_send()
        for b in range(B_LOC):
            for d in (1, 2, 3):
                ag_copy(d, b).wait_send()

    return pl.pallas_call(
        body,
        out_shape=jax.ShapeDtypeStruct((B_LOC, SQ, D), jnp.float32),
        in_specs=[pl.BlockSpec(memory_space=pl.ANY)] * 5,
        out_specs=pl.BlockSpec(memory_space=pltpu.VMEM),
        scratch_shapes=[
            pltpu.VMEM((B_LOC, SQ, D), jnp.float32),
            pltpu.VMEM((N_DEV, B_LOC, SQ, D), jnp.bfloat16),
            pltpu.VMEM((4, D, D), jnp.float32),
            pltpu.VMEM((4, D, D), jnp.bfloat16),
            pltpu.VMEM((4, SQ, DH), jnp.float32),
            pltpu.VMEM((8, SQ, D), jnp.bfloat16),
            pltpu.VMEM((6, SQ, D), jnp.bfloat16),
            pltpu.SemaphoreType.DMA((6,)),
            pltpu.SemaphoreType.DMA((6,)),
            pltpu.SemaphoreType.DMA((6,)),
            pltpu.SemaphoreType.DMA((6,)),
            pltpu.SemaphoreType.DMA((6,)),
        ],
        compiler_params=pltpu.CompilerParams(vmem_limit_bytes=110 * 1024 * 1024),
    )(x, Wq, Wk, Wv, Wo)
```
